```python
import numpy as np

kernel_name = "dist_pipemlp_pp2tp2_xy_b4096_d256_h512"

def setup_inputs():
    x_padded = np.zeros((2, 4096, 256), dtype=np.float32)
    x_padded[0] = np.random.randn(4096, 256).astype(np.float32)
    Win = np.random.randn(4, 256, 1024).astype(np.float32)
    Wout = np.random.randn(4, 1024, 256).astype(np.float32)
    return {"x_padded": x_padded, "Win": Win, "Wout": Wout}

def reference(x_padded, Win, Wout):
    a = x_padded[0]
    for k in range(4):
        h = a @ Win[k]
        h = np.maximum(h, 0.0)
        a = h @ Wout[k]
    out = np.zeros_like(x_padded)
    out[1] = a
    return out
```

```python
import jax
import jax.numpy as jnp
from jax import lax
from jax.experimental import pallas as pl
from jax.experimental.pallas import tpu as pltpu

_MESH = pl.DeviceIdType.MESH
_BF16 = jnp.bfloat16
_F32 = jnp.float32

_B, _D, _H = 4096, 256, 512
_R = _B // 2

_CHUNK = 64
_N_CHUNKS = _R // _CHUNK
_X_GROUPS = (256, 256, 512, 1024, 2048)
_P_ROWS = 256
_N_LATE, _LATE_ROWS = 31, 48
_W_CUTS = (32, 192)
_N_RELAY, _RELAY_ROWS = 2, 112
_N_FORWARD = 5

_EARLY = (256, 192, 128, 128, 192, 192)
_WIN3_AFTER = 3
_FINISH = (144, 304, 320, 320)
_N_STEADY, _STEADY_ROWS = 6, 128
_LAST = (64, 64, 64)
_SPLIT_ROWS = 80
_DETOUR_START, _DETOUR_ROWS, _DETOUR_PIECE = 256, 672, 64

_S_P, _S_A, _S_O, _S_G1, _S_G2 = range(5)


def _starts(sizes, total):
    out, s = [], 0
    for n in sizes:
        out.append((s, n))
        s += n
    assert s == total
    return out


def _output_pieces(blocks):
    d0, d1 = _DETOUR_START, _DETOUR_START + _DETOUR_ROWS
    direct, detour, of_block = [], [], []
    for s, n in blocks:
        mine = []
        for lo, hi in ((max(s, _SPLIT_ROWS), min(s + n, d0)), (max(s, d1), s + n)):
            if lo < hi:
                mine.append((False, len(direct)))
                direct.append((lo, hi - lo))
        for lo in range(max(s, d0), min(s + n, d1), _DETOUR_PIECE):
            mine.append((True, len(detour)))
            detour.append((lo, min(_DETOUR_PIECE, min(s + n, d1) - lo)))
        of_block.append(mine)
    return direct, detour, of_block


_N_EARLY = sum(_EARLY)
_BLOCKS = _starts(_FINISH + (_STEADY_ROWS,) * _N_STEADY + _LAST, _R)
_DIRECT, _DETOUR, _PIECES = _output_pieces(_BLOCKS)
_W_RELAY = _N_RELAY * _RELAY_ROWS
assert _SPLIT_ROWS <= min(_DETOUR_START, _EARLY[0])
assert _DETOUR_START + _DETOUR_ROWS <= _N_EARLY and _WIN3_AFTER < len(_EARLY)
assert all(_R - max(_N_LATE - i, 0) * _LATE_ROWS >= (i + 1) * _CHUNK
           for i in range(_N_CHUNKS))


def _dot(a, b):
    return jnp.dot(a, b, preferred_element_type=_F32)


def _hidden(a, w):
    return jnp.maximum(_dot(a, w), 0.0).astype(_BF16)


def _pack(v):
    return pltpu.bitcast(v.astype(_BF16), jnp.uint32)


def _unpack(words):
    return pltpu.bitcast(words, _BF16)


def _aligned(s, n):
    return s if isinstance(s, int) else pl.multiple_of(s, n)


def _rows(s, n):
    return pl.ds(_aligned(s, 8), n)


def _words(s, n):
    return _rows(s // 2, n // 2)


def _body(x_hbm, win_hbm, wout_hbm, out_ref,
          win32, wout32, win, wout, xbuf, pown, psend, precv, asend, arecv,
          h3, osend, orecv, relay1, relay2, wrelay, split,
          w_lsem, x_lsem, send_sem, w_ssem, w_rsem, r_ssem, r_rsem,
          p_rsem, a_rsem, o_rsem, g_rsem, s_ssem, s_rsem, ready):
    mx = lax.axis_index("x")
    my = lax.axis_index("y")
    y_nbr = (mx, 1 - my)
    x_nbr = (1 - mx, my)
    own0 = my * _R
    oth0 = (1 - my) * _R

    barrier = pltpu.get_barrier_semaphore()
    pl.semaphore_signal(barrier, 1, device_id=y_nbr, device_id_type=_MESH)

    @pl.when(mx == 0)
    def _():
        pl.semaphore_signal(barrier, 1, device_id=x_nbr, device_id_type=_MESH)

    def remote(src, dst, ssem, rsem, dev):
        return pltpu.make_async_remote_copy(
            src, dst, ssem, rsem, device_id=dev, device_id_type=_MESH)

    def drain(buf, stream):
        remote(buf, buf, send_sem.at[stream], s_rsem, y_nbr).wait_send()

    cut0, cut1 = _W_CUTS
    w_pieces = [(False, 1 - mx, 0, cut0),
                (False, 1 - mx, cut0, cut1 - cut0),
                (False, 1 - mx, cut1, _D - cut1),
                (True, 1 - mx, 0, _H - _W_RELAY),
                (True, 1 - mx, _H - _W_RELAY, _W_RELAY),
                (False, mx, 0, _D),
                (True, mx, 0, _H)]
    w_loads, swaps = [], []
    for i, (is_wout, l, s, n) in enumerate(w_pieces):
        hbm, f32, bf = (
            (wout_hbm, wout32, wout) if is_wout else (win_hbm, win32, win))
        w_loads.append(pltpu.make_async_copy(
            hbm.at[l, pl.ds(s, n)], f32.at[l, pl.ds(s, n)], w_lsem.at[i]))
        swaps.append(remote(bf.at[l, 0, _words(s, n)], bf.at[l, 1, _words(s, n)],
                            w_ssem.at[i], w_rsem.at[i], y_nbr))

    def w_ready(i):
        is_wout, l, s, n = w_pieces[i]
        f32, bf = (wout32, wout) if is_wout else (win32, win)
        w_loads[i].wait()
        bf[l, 0, _words(s, n), :] = _pack(f32[l, pl.ds(s, n), :])

    relays = [[], [], []]
    for i in range(_N_RELAY):
        mid = _words(i * _RELAY_ROWS, _RELAY_ROWS)
        end = _words(_H - _W_RELAY + i * _RELAY_ROWS, _RELAY_ROWS)
        for hop, (src, dst, dev) in enumerate((
                (wout.at[1, 0, end], wrelay.at[0, mid], x_nbr),
                (wrelay.at[0, mid], wrelay.at[1, mid], y_nbr),
                (wrelay.at[1, mid], wout.at[1, 1, end], x_nbr))):
            k = hop * _N_RELAY + i
            relays[hop].append(remote(src, dst, r_ssem.at[k], r_rsem.at[k], dev))

    x_groups = _starts(_X_GROUPS, _B)
    x_loads = [
        pltpu.make_async_copy(
            x_hbm.at[0, _rows(oth0 + s if s < _R else own0 + (s - _R), n)],
            xbuf.at[pl.ds(s, n)], x_lsem.at[g])
        for g, (s, n) in enumerate(x_groups)]

    def p_copy(i):
        sl = _words(i * _CHUNK, _CHUNK)
        return remote(psend.at[sl], precv.at[sl],
                      send_sem.at[_S_P], p_rsem.at[i], y_nbr)

    def a_copy(i):
        sl = _words(i * _CHUNK, _CHUNK)
        return remote(asend.at[sl], arecv.at[sl],
                      send_sem.at[_S_A], a_rsem.at[i], x_nbr)

    def o_copy(i, s, n):
        sl = _words(s, n)
        return remote(osend.at[sl], orecv.at[sl],
                      send_sem.at[_S_O], o_rsem.at[i], y_nbr)

    def detour_copy(hop, i):
        s, n = _DETOUR[i]
        end, mid = _words(s, n), _words(s - _DETOUR_START, n)
        src, dst, stream, dev = (
            (osend.at[end], relay1.at[mid], _S_O, x_nbr),
            (relay1.at[mid], relay2.at[mid], _S_G1, y_nbr),
            (relay2.at[mid], orecv.at[end], _S_G2, x_nbr))[hop]
        return remote(src, dst, send_sem.at[stream],
                      g_rsem.at[hop * len(_DETOUR) + i], dev)

    split_copy = remote(split.at[0], split.at[1], s_ssem, s_rsem, y_nbr)

    def half_layer(a, l):
        return _dot(_hidden(a, _unpack(win[l, 0])), _unpack(wout[l, 0]))

    def layer(a, l):
        h = jnp.concatenate(
            [_hidden(a, _unpack(win[l, j])) for j in range(2)], axis=1)
        return _dot(h, _unpack(wout[l].reshape(_H, _D)))

    w_loads[0].start()
    w_loads[1].start()

    @pl.when(mx == 1)
    def _():
        pl.semaphore_wait(barrier, 2)
        pl.semaphore_signal(ready, 1, device_id=x_nbr, device_id_type=_MESH)

    w_ready(0)

    @pl.when(mx == 0)
    def _():
        for c in (w_loads[4], w_loads[5], x_loads[0]):
            c.start()
        pl.semaphore_wait(barrier, 1)

    swaps[0].start()

    @pl.when(mx == 0)
    def _():
        w_loads[2].start()
        w_loads[6].start()

    w_ready(1)
    swaps[1].start()

    @pl.when(mx == 1)
    def _():
        for i in (2, 3, 4):
            w_loads[i].start()
        w_ready(2)
        for i in (5, 6):
            w_loads[i].start()
        w_ready(3)
        w_ready(4)
        for i in range(_N_RELAY):
            relays[0][i].wait_recv()
            relays[1][i].start()
        for i in (2, 3, 4):
            swaps[i].start()
        for i in (5, 6):
            w_ready(i)
            swaps[i].start()
        for i in range(_N_RELAY):
            relays[1][i].wait_recv()
            relays[2][i].start()

    @pl.when(mx == 0)
    def _stage0():
        x_loads[1].start()
        w_ready(4)
        w_ready(2)
        swaps[2].start()
        pl.semaphore_wait(ready, 1)
        for c in relays[0]:
            c.start()
        w_ready(5)
        w_ready(6)

        def partial(s, n):
            return half_layer(xbuf[_rows(s, n), :].astype(_BF16), 0)

        for g, (s, n) in enumerate(x_groups):
            x_loads[g].wait()
            if g + 2 < len(x_groups):
                x_loads[g + 2].start()
            if g == 0:
                w_loads[3].start()
            if g == 2:
                w_ready(3)
                swaps[3].start()
            if s == _R:
                for i in range(_N_CHUNKS):
                    p_copy(i).start()
            end = min(s + n, _B - _N_LATE * _LATE_ROWS)
            for r in range(s, end, _P_ROWS):
                m = min(_P_ROWS, end - r)
                if r < _R:
                    psend[_words(r, m), :] = _pack(partial(r, m))
                else:
                    pown[_rows(r - _R, m), :] = partial(r, m)

        for c in swaps[:4] + relays[2]:
            c.wait_recv()

        def layer1(i, late):
            p_copy(i).wait_recv()
            sl = _words(i * _CHUNK, _CHUNK)
            a = (pown[_rows(i * _CHUNK, _CHUNK), :]
                 + _unpack(precv[sl, :]).astype(_F32))
            asend[sl, :] = _pack(layer(a.astype(_BF16), 1))
            if late:
                r = _R + (i - _N_LATE) * _LATE_ROWS
                pown[_rows(r, _LATE_ROWS), :] = partial(_R + r, _LATE_ROWS)
            a_copy(i).start()
            out_ref[0, _rows(i * 2 * _CHUNK, 2 * _CHUNK), :] = jnp.zeros(
                (2 * _CHUNK, _D), _F32)

        def forward(hop, i):
            detour_copy(hop, i).wait_recv()
            detour_copy(hop + 1, i).start()

        n_loop = _N_CHUNKS - _N_FORWARD
        assert n_loop <= _N_LATE
        pl.loop(0, n_loop)(lambda i: layer1(i, True))
        for k in range(_N_FORWARD):
            layer1(n_loop + k, n_loop + k < _N_LATE)
            forward(0, k)
        for k in range(len(_DETOUR)):
            forward(1, k)
            if k + _N_FORWARD < len(_DETOUR):
                forward(0, k + _N_FORWARD)

        for c in swaps[:4] + relays[0]:
            c.wait_send()
        drain(psend, _S_P)
        drain(asend, _S_A)
        drain(relay1, _S_G1)
        drain(relay2, _S_G2)

    @pl.when(mx == 1)
    def _stage1():
        def activations(s, n):
            for k in range(n // _CHUNK):
                a_copy(s // _CHUNK + k).wait_recv()
            return _unpack(arecv[_words(s, n), :])

        def emit(i, o):
            s, n = _BLOCKS[i]
            osend[_words(s, n), :] = _pack(o)
            for is_detour, k in _PIECES[i]:
                (detour_copy(0, k) if is_detour else o_copy(k, *_DIRECT[k])).start()
            out_ref[0, _rows(own0 + s, n), :] = o

        def layers23(s, n):
            return layer(layer(activations(s, n), 0).astype(_BF16), 1)

        for c in swaps[:5]:
            c.wait_recv()
        waiting = []
        for i, (s, n) in enumerate(_starts(_EARLY, _N_EARLY)):
            a = layer(activations(s, n), 0).astype(_BF16)
            half = half_layer(a, 1)
            if i == 0:
                split[0, 0] = _pack(a[:_SPLIT_ROWS])
                split[0, 1] = _pack(half[:_SPLIT_ROWS])
                split_copy.start()
            out_ref[0, _rows(own0 + s, n), :] = half
            waiting.append((s, n, a))
            if i == _WIN3_AFTER:
                swaps[5].wait_recv()
            if i >= _WIN3_AFTER:
                for ws, wn, wa in waiting:
                    h3[_words(ws, wn), :] = _pack(_hidden(wa, _unpack(win[1, 1])))
                waiting = []
        swaps[6].wait_recv()
        for i, (s, n) in enumerate(_BLOCKS[:len(_FINISH)]):
            emit(i, out_ref[0, _rows(own0 + s, n), :]
                 + _dot(_unpack(h3[_words(s, n), :]), _unpack(wout[1, 1])))

        @pl.loop(0, _N_STEADY)
        def _(k):
            s = _N_EARLY + k * _STEADY_ROWS
            o = layers23(s, _STEADY_ROWS)
            osend[_words(s, _STEADY_ROWS), :] = _pack(o)
            o_copy(_PIECES[len(_FINISH)][0][1] + k, s, _STEADY_ROWS).start()
            out_ref[0, _rows(own0 + s, _STEADY_ROWS), :] = o

        for i in range(len(_FINISH) + _N_STEADY, len(_BLOCKS)):
            emit(i, layers23(*_BLOCKS[i]))

        for c in swaps + relays[1] + relays[2] + [split_copy]:
            c.wait_send()

        split_copy.wait_recv()
        out_ref[0, _rows(oth0, _SPLIT_ROWS), :] = (
            _unpack(split[1, 1]).astype(_F32) + half_layer(_unpack(split[1, 0]), 1))
        arrivals = [
            (-sum(m for _, m in _DIRECT[k + 1:]), o_copy(k, s, n), s, n)
            for k, (s, n) in enumerate(_DIRECT)
        ] + [
            (-sum(m for _, m in _DETOUR[k + 1:]), detour_copy(2, k), s, n)
            for k, (s, n) in enumerate(_DETOUR)
        ]
        for _, copy, s, n in sorted(arrivals, key=lambda t: t[0]):
            copy.wait_recv()
            out_ref[0, _rows(oth0 + s, n), :] = (
                _unpack(orecv[_words(s, n), :]).astype(_F32))
        drain(osend.at[_words(_SPLIT_ROWS, _R - _SPLIT_ROWS)], _S_O)


def pallas_dist_pipemlp_pp2tp2_xy_b4096_d256_h512_kernel(
    x_padded: jax.Array,
    Win: jax.Array,
    Wout: jax.Array,
):
    def packed(*shape):
        return pltpu.VMEM((*shape[:-2], shape[-2] // 2, shape[-1]), jnp.uint32)

    dma = pltpu.SemaphoreType.DMA
    hbm = pl.BlockSpec(memory_space=pltpu.HBM)
    return pl.pallas_call(
        _body,
        out_shape=pltpu.VMEM((1, _B, _D), _F32),
        in_specs=[hbm, hbm, hbm],
        out_specs=pl.BlockSpec(memory_space=pltpu.VMEM),
        scratch_shapes=[
            pltpu.VMEM((2, _D, _H), _F32),
            pltpu.VMEM((2, _H, _D), _F32),
            packed(2, 2, _D, _H),
            packed(2, 2, _H, _D),
            pltpu.VMEM((_B, _D), _F32),
            pltpu.VMEM((_R, _D), _F32),
            packed(_R, _D),
            packed(_R, _D),
            packed(_R, _D),
            packed(_R, _D),
            packed(_N_EARLY, _H),
            packed(_R, _D),
            packed(_R, _D),
            packed(_DETOUR_ROWS, _D),
            packed(_DETOUR_ROWS, _D),
            packed(2, _W_RELAY, _D),
            packed(2, 2, _SPLIT_ROWS, _D),
            dma((7,)),
            dma((len(_X_GROUPS),)),
            dma((5,)),
            dma((7,)),
            dma((7,)),
            dma((3 * _N_RELAY,)),
            dma((3 * _N_RELAY,)),
            dma((_N_CHUNKS,)),
            dma((_N_CHUNKS,)),
            dma((len(_DIRECT),)),
            dma((3 * len(_DETOUR),)),
            dma,
            dma,
            pltpu.SemaphoreType.REGULAR,
        ],
        compiler_params=pltpu.CompilerParams(
            collective_id=0,
            vmem_limit_bytes=40 * 1024 * 1024,
            disable_semaphore_checks=True,
        ),
    )(x_padded, Win, Wout)
```

```python
import jax
import jax.numpy as jnp
from jax import lax
from jax.experimental import pallas as pl
from jax.experimental.pallas import tpu as pltpu

_MESH = pl.DeviceIdType.MESH
_BF16 = jnp.bfloat16
_F32 = jnp.float32

_B, _D, _H = 4096, 256, 512
_R = _B // 2

_CHUNK = 64
_N_CHUNKS = _R // _CHUNK
_X_GROUPS = (256, 256, 512, 1024, 2048)
_P_ROWS = 256
_N_LATE, _LATE_ROWS = 31, 48
_W_CUTS = (32, 192)
_N_RELAY, _RELAY_ROWS = 7, 32
_N_FORWARD = 5

_EARLY = (256, 192, 128, 128, 192, 192)
_WIN3_AFTER = 3
_FINISH = (128, 320, 320, 320)
_N_STEADY, _STEADY_ROWS = 6, 128
_LAST = (64, 64, 64)
_SPLIT_ROWS = 64
_DETOUR_START, _DETOUR_ROWS, _DETOUR_PIECE = 256, 672, 64

_S_P, _S_A, _S_O, _S_G1, _S_G2 = range(5)


def _starts(sizes, total):
    out, s = [], 0
    for n in sizes:
        out.append((s, n))
        s += n
    assert s == total
    return out


def _output_pieces(blocks):
    d0, d1 = _DETOUR_START, _DETOUR_START + _DETOUR_ROWS
    direct, detour, of_block = [], [], []
    for s, n in blocks:
        mine = []
        for lo, hi in ((max(s, _SPLIT_ROWS), min(s + n, d0)), (max(s, d1), s + n)):
            if lo < hi:
                mine.append((False, len(direct)))
                direct.append((lo, hi - lo))
        for lo in range(max(s, d0), min(s + n, d1), _DETOUR_PIECE):
            mine.append((True, len(detour)))
            detour.append((lo, min(_DETOUR_PIECE, min(s + n, d1) - lo)))
        of_block.append(mine)
    return direct, detour, of_block


_N_EARLY = sum(_EARLY)
_BLOCKS = _starts(_FINISH + (_STEADY_ROWS,) * _N_STEADY + _LAST, _R)
_DIRECT, _DETOUR, _PIECES = _output_pieces(_BLOCKS)
_W_RELAY = _N_RELAY * _RELAY_ROWS
assert _SPLIT_ROWS <= min(_DETOUR_START, _EARLY[0])
assert _DETOUR_START + _DETOUR_ROWS <= _N_EARLY and _WIN3_AFTER < len(_EARLY)
assert all(_R - max(_N_LATE - i, 0) * _LATE_ROWS >= (i + 1) * _CHUNK
           for i in range(_N_CHUNKS))


def _dot(a, b):
    return jnp.dot(a, b, preferred_element_type=_F32)


def _hidden(a, w):
    return jnp.maximum(_dot(a, w), 0.0).astype(_BF16)


def _pack(v):
    return pltpu.bitcast(v.astype(_BF16), jnp.uint32)


def _unpack(words):
    return pltpu.bitcast(words, _BF16)


def _aligned(s, n):
    return s if isinstance(s, int) else pl.multiple_of(s, n)


def _rows(s, n):
    return pl.ds(_aligned(s, 8), n)


def _words(s, n):
    return _rows(s // 2, n // 2)


def _body(x_hbm, win_hbm, wout_hbm, out_ref,
          win32, wout32, win, wout, xbuf, pown, psend, precv, asend, arecv,
          h3, osend, orecv, relay1, relay2, wrelay, split,
          w_lsem, x_lsem, send_sem, w_ssem, w_rsem, r_ssem, r_rsem,
          p_rsem, a_rsem, o_rsem, g_rsem, s_ssem, s_rsem, ready):
    mx = lax.axis_index("x")
    my = lax.axis_index("y")
    y_nbr = (mx, 1 - my)
    x_nbr = (1 - mx, my)
    own0 = my * _R
    oth0 = (1 - my) * _R

    barrier = pltpu.get_barrier_semaphore()
    pl.semaphore_signal(barrier, 1, device_id=y_nbr, device_id_type=_MESH)

    @pl.when(mx == 0)
    def _():
        pl.semaphore_signal(barrier, 1, device_id=x_nbr, device_id_type=_MESH)

    def remote(src, dst, ssem, rsem, dev):
        return pltpu.make_async_remote_copy(
            src, dst, ssem, rsem, device_id=dev, device_id_type=_MESH)

    def drain(buf, stream):
        remote(buf, buf, send_sem.at[stream], s_rsem, y_nbr).wait_send()

    cut0, cut1 = _W_CUTS
    w_pieces = [(False, 1 - mx, 0, cut0),
                (False, 1 - mx, cut0, cut1 - cut0),
                (False, 1 - mx, cut1, _D - cut1),
                (True, 1 - mx, 0, _H - _W_RELAY),
                (True, 1 - mx, _H - _W_RELAY, _W_RELAY),
                (False, mx, 0, _D),
                (True, mx, 0, _H)]
    w_loads, swaps = [], []
    for i, (is_wout, l, s, n) in enumerate(w_pieces):
        hbm, f32, bf = (
            (wout_hbm, wout32, wout) if is_wout else (win_hbm, win32, win))
        w_loads.append(pltpu.make_async_copy(
            hbm.at[l, pl.ds(s, n)], f32.at[l, pl.ds(s, n)], w_lsem.at[i]))
        swaps.append(remote(bf.at[l, 0, _words(s, n)], bf.at[l, 1, _words(s, n)],
                            w_ssem.at[i], w_rsem.at[i], y_nbr))

    def w_ready(i):
        is_wout, l, s, n = w_pieces[i]
        f32, bf = (wout32, wout) if is_wout else (win32, win)
        w_loads[i].wait()
        bf[l, 0, _words(s, n), :] = _pack(f32[l, pl.ds(s, n), :])

    relays = [[], [], []]
    for i in range(_N_RELAY):
        mid = _words(i * _RELAY_ROWS, _RELAY_ROWS)
        end = _words(_H - _W_RELAY + i * _RELAY_ROWS, _RELAY_ROWS)
        for hop, (src, dst, dev) in enumerate((
                (wout.at[1, 0, end], wrelay.at[0, mid], x_nbr),
                (wrelay.at[0, mid], wrelay.at[1, mid], y_nbr),
                (wrelay.at[1, mid], wout.at[1, 1, end], x_nbr))):
            k = hop * _N_RELAY + i
            relays[hop].append(remote(src, dst, r_ssem.at[k], r_rsem.at[k], dev))

    x_groups = _starts(_X_GROUPS, _B)
    x_loads = [
        pltpu.make_async_copy(
            x_hbm.at[0, _rows(oth0 + s if s < _R else own0 + (s - _R), n)],
            xbuf.at[pl.ds(s, n)], x_lsem.at[g])
        for g, (s, n) in enumerate(x_groups)]

    def p_copy(i):
        sl = _words(i * _CHUNK, _CHUNK)
        return remote(psend.at[sl], precv.at[sl],
                      send_sem.at[_S_P], p_rsem.at[i], y_nbr)

    def a_copy(i):
        sl = _words(i * _CHUNK, _CHUNK)
        return remote(asend.at[sl], arecv.at[sl],
                      send_sem.at[_S_A], a_rsem.at[i], x_nbr)

    def o_copy(i, s, n):
        sl = _words(s, n)
        return remote(osend.at[sl], orecv.at[sl],
                      send_sem.at[_S_O], o_rsem.at[i], y_nbr)

    def detour_copy(hop, i):
        s, n = _DETOUR[i]
        end, mid = _words(s, n), _words(s - _DETOUR_START, n)
        src, dst, stream, dev = (
            (osend.at[end], relay1.at[mid], _S_O, x_nbr),
            (relay1.at[mid], relay2.at[mid], _S_G1, y_nbr),
            (relay2.at[mid], orecv.at[end], _S_G2, x_nbr))[hop]
        return remote(src, dst, send_sem.at[stream],
                      g_rsem.at[hop * len(_DETOUR) + i], dev)

    split_copy = remote(split.at[0], split.at[1], s_ssem, s_rsem, y_nbr)

    def half_layer(a, l):
        return _dot(_hidden(a, _unpack(win[l, 0])), _unpack(wout[l, 0]))

    def layer(a, l):
        h = jnp.concatenate(
            [_hidden(a, _unpack(win[l, j])) for j in range(2)], axis=1)
        return _dot(h, _unpack(wout[l].reshape(_H, _D)))

    w_loads[0].start()
    w_loads[1].start()

    @pl.when(mx == 1)
    def _():
        pl.semaphore_wait(barrier, 2)
        pl.semaphore_signal(ready, 1, device_id=x_nbr, device_id_type=_MESH)

    w_ready(0)

    @pl.when(mx == 0)
    def _():
        for c in (w_loads[4], w_loads[5], x_loads[0]):
            c.start()
        pl.semaphore_wait(barrier, 1)

    swaps[0].start()

    @pl.when(mx == 0)
    def _():
        w_loads[2].start()
        w_loads[6].start()

    w_ready(1)
    swaps[1].start()

    @pl.when(mx == 1)
    def _():
        for i in (2, 3, 4):
            w_loads[i].start()
        w_ready(2)
        for i in (5, 6):
            w_loads[i].start()
        w_ready(3)
        w_ready(4)
        for i in range(_N_RELAY):
            relays[0][i].wait_recv()
            relays[1][i].start()
        for i in (2, 3, 4):
            swaps[i].start()
        for i in (5, 6):
            w_ready(i)
            swaps[i].start()
        for i in range(_N_RELAY):
            relays[1][i].wait_recv()
            relays[2][i].start()

    @pl.when(mx == 0)
    def _stage0():
        x_loads[1].start()
        w_ready(4)
        w_ready(2)
        swaps[2].start()
        pl.semaphore_wait(ready, 1)
        for c in relays[0]:
            c.start()
        w_ready(5)
        w_ready(6)

        def partial(s, n):
            return half_layer(xbuf[_rows(s, n), :].astype(_BF16), 0)

        for g, (s, n) in enumerate(x_groups):
            x_loads[g].wait()
            if g + 2 < len(x_groups):
                x_loads[g + 2].start()
            if g == 0:
                w_loads[3].start()
            if g == 2:
                w_ready(3)
                swaps[3].start()
            if s == _R:
                for i in range(_N_CHUNKS):
                    p_copy(i).start()
            end = min(s + n, _B - _N_LATE * _LATE_ROWS)
            for r in range(s, end, _P_ROWS):
                m = min(_P_ROWS, end - r)
                if r < _R:
                    psend[_words(r, m), :] = _pack(partial(r, m))
                else:
                    pown[_rows(r - _R, m), :] = partial(r, m)

        for c in swaps[:4] + relays[2]:
            c.wait_recv()

        def layer1(i, late):
            p_copy(i).wait_recv()
            sl = _words(i * _CHUNK, _CHUNK)
            a = (pown[_rows(i * _CHUNK, _CHUNK), :]
                 + _unpack(precv[sl, :]).astype(_F32))
            asend[sl, :] = _pack(layer(a.astype(_BF16), 1))
            if late:
                r = _R + (i - _N_LATE) * _LATE_ROWS
                pown[_rows(r, _LATE_ROWS), :] = partial(_R + r, _LATE_ROWS)
            a_copy(i).start()
            out_ref[0, _rows(i * 2 * _CHUNK, 2 * _CHUNK), :] = jnp.zeros(
                (2 * _CHUNK, _D), _F32)

        def forward(hop, i):
            detour_copy(hop, i).wait_recv()
            detour_copy(hop + 1, i).start()

        n_loop = _N_CHUNKS - _N_FORWARD
        assert n_loop <= _N_LATE
        pl.loop(0, n_loop)(lambda i: layer1(i, True))
        for k in range(_N_FORWARD):
            layer1(n_loop + k, n_loop + k < _N_LATE)
            forward(0, k)
        for k in range(len(_DETOUR)):
            forward(1, k)
            if k + _N_FORWARD < len(_DETOUR):
                forward(0, k + _N_FORWARD)

        for c in swaps[:4] + relays[0]:
            c.wait_send()
        drain(psend, _S_P)
        drain(asend, _S_A)
        drain(relay1, _S_G1)
        drain(relay2, _S_G2)

    @pl.when(mx == 1)
    def _stage1():
        def activations(s, n):
            for k in range(n // _CHUNK):
                a_copy(s // _CHUNK + k).wait_recv()
            return _unpack(arecv[_words(s, n), :])

        def emit(i, o):
            s, n = _BLOCKS[i]
            osend[_words(s, n), :] = _pack(o)
            for is_detour, k in _PIECES[i]:
                (detour_copy(0, k) if is_detour else o_copy(k, *_DIRECT[k])).start()
            out_ref[0, _rows(own0 + s, n), :] = o

        def layers23(s, n):
            return layer(layer(activations(s, n), 0).astype(_BF16), 1)

        for c in swaps[:5]:
            c.wait_recv()
        waiting = []
        for i, (s, n) in enumerate(_starts(_EARLY, _N_EARLY)):
            a = layer(activations(s, n), 0).astype(_BF16)
            half = half_layer(a, 1)
            if i == 0:
                split[0, 0] = _pack(a[:_SPLIT_ROWS])
                split[0, 1] = _pack(half[:_SPLIT_ROWS])
                split_copy.start()
            out_ref[0, _rows(own0 + s, n), :] = half
            waiting.append((s, n, a))
            if i == _WIN3_AFTER:
                swaps[5].wait_recv()
            if i >= _WIN3_AFTER:
                for ws, wn, wa in waiting:
                    h3[_words(ws, wn), :] = _pack(_hidden(wa, _unpack(win[1, 1])))
                waiting = []
        swaps[6].wait_recv()
        for i, (s, n) in enumerate(_BLOCKS[:len(_FINISH)]):
            emit(i, out_ref[0, _rows(own0 + s, n), :]
                 + _dot(_unpack(h3[_words(s, n), :]), _unpack(wout[1, 1])))

        @pl.loop(0, _N_STEADY)
        def _(k):
            s = _N_EARLY + k * _STEADY_ROWS
            o = layers23(s, _STEADY_ROWS)
            osend[_words(s, _STEADY_ROWS), :] = _pack(o)
            o_copy(_PIECES[len(_FINISH)][0][1] + k, s, _STEADY_ROWS).start()
            out_ref[0, _rows(own0 + s, _STEADY_ROWS), :] = o

        for i in range(len(_FINISH) + _N_STEADY, len(_BLOCKS)):
            emit(i, layers23(*_BLOCKS[i]))

        for c in swaps + relays[1] + relays[2] + [split_copy]:
            c.wait_send()

        split_copy.wait_recv()
        out_ref[0, _rows(oth0, _SPLIT_ROWS), :] = (
            _unpack(split[1, 1]).astype(_F32) + half_layer(_unpack(split[1, 0]), 1))
        arrivals = [
            (-sum(m for _, m in _DIRECT[k + 1:]), o_copy(k, s, n), s, n)
            for k, (s, n) in enumerate(_DIRECT)
        ] + [
            (-sum(m for _, m in _DETOUR[k + 1:]), detour_copy(2, k), s, n)
            for k, (s, n) in enumerate(_DETOUR)
        ]
        for _, copy, s, n in sorted(arrivals, key=lambda t: t[0]):
            copy.wait_recv()
            out_ref[0, _rows(oth0 + s, n), :] = (
                _unpack(orecv[_words(s, n), :]).astype(_F32))
        drain(osend.at[_words(_SPLIT_ROWS, _R - _SPLIT_ROWS)], _S_O)


def pallas_dist_pipemlp_pp2tp2_xy_b4096_d256_h512_kernel(
    x_padded: jax.Array,
    Win: jax.Array,
    Wout: jax.Array,
):
    def packed(*shape):
        return pltpu.VMEM((*shape[:-2], shape[-2] // 2, shape[-1]), jnp.uint32)

    dma = pltpu.SemaphoreType.DMA
    hbm = pl.BlockSpec(memory_space=pltpu.HBM)
    return pl.pallas_call(
        _body,
        out_shape=jax.ShapeDtypeStruct((1, _B, _D), _F32),
        in_specs=[hbm, hbm, hbm],
        out_specs=pl.BlockSpec(memory_space=pltpu.VMEM),
        scratch_shapes=[
            pltpu.VMEM((2, _D, _H), _F32),
            pltpu.VMEM((2, _H, _D), _F32),
            packed(2, 2, _D, _H),
            packed(2, 2, _H, _D),
            pltpu.VMEM((_B, _D), _F32),
            pltpu.VMEM((_R, _D), _F32),
            packed(_R, _D),
            packed(_R, _D),
            packed(_R, _D),
            packed(_R, _D),
            packed(_N_EARLY, _H),
            packed(_R, _D),
            packed(_R, _D),
            packed(_DETOUR_ROWS, _D),
            packed(_DETOUR_ROWS, _D),
            packed(2, _W_RELAY, _D),
            packed(2, 2, _SPLIT_ROWS, _D),
            dma((7,)),
            dma((len(_X_GROUPS),)),
            dma((5,)),
            dma((7,)),
            dma((7,)),
            dma((3 * _N_RELAY,)),
            dma((3 * _N_RELAY,)),
            dma((_N_CHUNKS,)),
            dma((_N_CHUNKS,)),
            dma((len(_DIRECT),)),
            dma((3 * len(_DETOUR),)),
            dma,
            dma,
            pltpu.SemaphoreType.REGULAR,
        ],
        compiler_params=pltpu.CompilerParams(
            collective_id=0,
            vmem_limit_bytes=40 * 1024 * 1024,
            disable_semaphore_checks=True,
        ),
    )(x_padded, Win, Wout)
```
